```python
import numpy as np

kernel_name = "dist_ar_xy_y_m256_n256"

def setup_inputs():
    return {"x": np.random.randn(512, 256).astype(np.float32)}

def reference(x: np.ndarray) -> np.ndarray:
    return x.reshape(2, 256, 256).sum(axis=0)
```

```python
import functools

import jax
import jax.numpy as jnp
from jax import lax
from jax.experimental import pallas as pl
from jax.experimental.pallas import tpu as pltpu

_MESH = pl.DeviceIdType.MESH
_DEV = {"A": (0, 0), "B": (1, 0), "C": (0, 1), "D": (1, 1)}
_Y_PEER = {"A": "C", "C": "A", "B": "D", "D": "B"}
_X_PEER = {"A": "B", "B": "A", "C": "D", "D": "C"}
_NK = 64

_SENDS = {
    "C": [
        ("f", 0, 2, False), ("f", 2, 3, False),
        ("b", 3, 4, False), ("b", 4, 6, False), ("b", 6, 10, False),
        ("b", 10, 22, True), ("b", 22, 48, False), ("b", 48, 50, False),
        ("b", 50, 51, False), ("b", 51, 52, False),
    ],
    "D": [("f", 52, 53, True), ("f", 53, 54, True)]
    + [("b", k, k + 1, True) for k in range(54, 64)]
    + [("b", 0, 10, False), ("b", 22, 50, False), ("b", 50, 52, False)],
    "A": [("b", 0, 12, True), ("b", 12, 50, False), ("b", 50, 52, False)],
    "B": [
        ("b", 52, 58, True), ("b", 58, 64, True),
        ("b", 12, 50, False), ("b", 50, 52, False),
    ],
}
_LOADS = {
    "C": [(3, 4), (4, 6), (6, 10), (10, 22), (22, 64), (0, 2), (2, 3)],
    "D": [(54, 55), (55, 56), (56, 57), (57, 58), (58, 64), (0, 54)],
    "A": [(0, 64)],
    "B": [(0, 64)],
}
_ORDER_A = (
    [("y", i) for i in range(6)] + [None]
    + [("x", i) for i in range(8)]
    + [("y", 6), ("x", 8), ("x", 9), ("y", 7), ("x", 10), ("y", 8), ("x", 11), ("y", 9)]
)


def _recv_order(r):
    if r == "A":
        return _ORDER_A
    ys = [("y", i) for i in range(len(_SENDS[_Y_PEER[r]]))]
    diag = _SENDS[_Y_PEER[_X_PEER[r]]]
    xs = [("x", i) for i, msg in enumerate(diag) if msg[3]]
    return ys[:-1] + xs + ys[-1:]


def _tile(k):
    return pl.ds(8 * (k // 2), 8), pl.ds(128 * (k % 2), 128)


def _rect(ref, k0, k1):
    if k1 - k0 == 1:
        return ref.at[_tile(k0)]
    assert k0 % 2 == 0 and k1 % 2 == 0
    return ref.at[pl.ds(4 * k0, 4 * (k1 - k0))]


def _body(x_hbm, o_ref, xv, sbuf, rbuf, hbuf,
          y_send, y_recv, x_send, x_recv, load_sem, entry_sem):
    my_x = lax.axis_index("x")
    my_y = lax.axis_index("y")
    barrier = pltpu.get_barrier_semaphore()
    pl.semaphore_signal(barrier, inc=1, device_id=(my_x, 1 - my_y),
                        device_id_type=_MESH)

    def signal(sem, dev):
        pl.semaphore_signal(sem, inc=1, device_id=_DEV[dev], device_id_type=_MESH)

    def y_copy(msg, i, dev):
        kind, k0, k1, _ = msg
        if kind == "b":
            src, dst = sbuf.at[pl.ds(k0, k1 - k0)], rbuf.at[pl.ds(k0, k1 - k0)]
        else:
            src, dst = _rect(x_hbm, k0, k1), _rect(hbuf, k0, k1)
        return pltpu.make_async_remote_copy(
            src_ref=src, dst_ref=dst, send_sem=y_send.at[i], recv_sem=y_recv.at[i],
            device_id=_DEV[dev], device_id_type=_MESH)

    def x_copy(msg, i, dev):
        _, k0, k1, _ = msg
        buf = rbuf.at[pl.ds(k0, k1 - k0)]
        return pltpu.make_async_remote_copy(
            src_ref=buf, dst_ref=buf, send_sem=x_send.at[i], recv_sem=x_recv.at[i],
            device_id=_DEV[dev], device_id_type=_MESH)

    def add(kind, k0, k1):
        for k in range(k0, k1):
            t = _tile(k)
            other = rbuf[k].astype(jnp.float32) if kind == "b" else hbuf[t]
            o_ref[t] = xv[t] + other

    def program(r):
        yp, xp = _Y_PEER[r], _X_PEER[r]
        mine = _SENDS[r]
        n_head = sum(msg[0] == "f" for msg in mine)
        in_flight = []

        def wait_peers():
            pl.semaphore_wait(barrier, 1 if r == "C" else 2)

        def send(i):
            cp = y_copy(mine[i], i, yp)
            cp.start()
            in_flight.append(cp)

        if r != "D":
            signal(barrier, xp)
        if r == "C":
            wait_peers()
            for i in range(n_head):
                send(i)

        loads = []
        for i, (k0, k1) in enumerate(_LOADS[r]):
            cp = pltpu.make_async_copy(
                _rect(x_hbm, k0, k1), _rect(xv, k0, k1), load_sem.at[i])
            cp.start()
            loads.append(cp)

        if r == "D":
            wait_peers()
            for i in range(n_head):
                send(i)
            signal(entry_sem, "C")

        landed = set()

        def need(k0, k1):
            for i, (l0, l1) in enumerate(_LOADS[r]):
                if l0 < k1 and k0 < l1 and i not in landed:
                    loads[i].wait()
                    landed.add(i)

        def pack(i):
            _, k0, k1, _ = mine[i]
            need(k0, k1)
            for k in range(k0, k1):
                sbuf[k] = xv[_tile(k)].astype(jnp.bfloat16)

        if r in "AB":
            for i in range(n_head, len(mine)):
                pack(i)
            wait_peers()
            for i in range(n_head, len(mine)):
                send(i)
        else:
            for i in range(n_head, len(mine)):
                pack(i)
                send(i)
        need(0, _NK)

        if r == "C":
            pl.semaphore_wait(entry_sem, 1)

        from_y, from_diag = _SENDS[yp], _SENDS[_Y_PEER[xp]]
        deferred = []

        def flush():
            for kind, k0, k1, _ in deferred:
                add(kind, k0, k1)
            deferred.clear()

        def drain():
            for cp in in_flight:
                cp.wait_send()
            in_flight.clear()

        for event in _recv_order(r):
            if event is None:
                drain()
                continue
            src, i = event
            if src == "y":
                msg = from_y[i]
                kind, k0, k1, fwd = msg
                y_copy(msg, i, yp).wait_recv()
                if fwd:
                    if kind == "f":
                        for k in range(k0, k1):
                            rbuf[k] = hbuf[_tile(k)].astype(jnp.bfloat16)
                    cp = x_copy(msg, i, xp)
                    cp.start()
                    in_flight.append(cp)
                    deferred.append(msg)
                else:
                    flush()
                    add(kind, k0, k1)
            else:
                msg = from_diag[i]
                flush()
                x_copy(msg, i, xp).wait_recv()
                add("b", msg[1], msg[2])
        flush()
        drain()

    for r in "CDAB":
        is_r = jnp.logical_and(my_x == _DEV[r][0], my_y == _DEV[r][1])
        pl.when(is_r)(functools.partial(program, r))


def pallas_dist_ar_xy_y_m256_n256_kernel(x: jax.Array):
    m, n = x.shape
    assert (m, n) == (256, 256)
    n_msg = max(len(v) for v in _SENDS.values())
    n_load = max(len(v) for v in _LOADS.values())
    return pl.pallas_call(
        _body,
        out_shape=jax.ShapeDtypeStruct((m, n), x.dtype),
        in_specs=[pl.BlockSpec(memory_space=pl.ANY)],
        out_specs=pl.BlockSpec(memory_space=pltpu.VMEM),
        scratch_shapes=[
            pltpu.VMEM((m, n), x.dtype),
            pltpu.VMEM((_NK, 8, 128), jnp.bfloat16),
            pltpu.VMEM((_NK, 8, 128), jnp.bfloat16),
            pltpu.VMEM((m, n), x.dtype),
            pltpu.SemaphoreType.DMA((n_msg,)),
            pltpu.SemaphoreType.DMA((n_msg,)),
            pltpu.SemaphoreType.DMA((n_msg,)),
            pltpu.SemaphoreType.DMA((n_msg,)),
            pltpu.SemaphoreType.DMA((n_load,)),
            pltpu.SemaphoreType.REGULAR,
        ],
        compiler_params=pltpu.CompilerParams(
            collective_id=0,
            disable_bounds_checks=True,
            disable_semaphore_checks=True,
        ),
    )(x)
```

```python
import functools

import jax
import jax.numpy as jnp
from jax import lax
from jax.experimental import pallas as pl
from jax.experimental.pallas import tpu as pltpu

_MESH = pl.DeviceIdType.MESH
_DEV = {"A": (0, 0), "B": (1, 0), "C": (0, 1), "D": (1, 1)}
_Y_PEER = {"A": "C", "C": "A", "B": "D", "D": "B"}
_X_PEER = {"A": "B", "B": "A", "C": "D", "D": "C"}
_NG = 64

_X1 = [
    (14, 15, 0), (30, 31, 1), (42, 43, 1), (50, 51, 1),
    (0, 5, 0), (9, 12, 1), (17, 20, 1), (7, 22, 0), (25, 28, 0),
    (0, 5, 1), (2, 3, 0), 1, 4,
    (14, 15, 1), (9, 12, 0), 6, 8, 10, 11, 13,
    (30, 31, 0), (17, 20, 0), (7, 22, 1), (25, 28, 1),
    16, 18, 19, 21, 24, 26, 27, 29, 32, 34, 35,
    (42, 43, 0), (50, 51, 0), (58, 59, 1), (33, 36, 1), (23, 38, 0),
    (40, 45, 1), (48, 53, 1), (56, 61, 0), 37, 39, 41, 44, 46, 47, 49, 52, 54,
    (58, 59, 0), (2, 3, 1), (33, 36, 0), (23, 38, 1), (40, 45, 0), (48, 53, 0),
    (56, 61, 1), 55, 57, 60, 62, 63,
]

_SENDS = {
    "C": [
        ("f", 0, 2, False), ("f", 2, 4, False), ("f", 4, 6, False),
        ("b", 6, 8, False), ("b", 8, 10, False), ("b", 10, 12, False),
        ("b", 12, 18, False), ("b", 18, 26, True), ("b", 26, 40, True),
        ("b", 40, 70, False), ("b", 70, 96, False), ("b", 96, 100, False),
        ("b", 100, 102, False), ("b", 102, 103, False),
    ],
    "D": [("f", h, h + 1, True) for h in range(104, 108)]
    + [("b", h, h + 1, True) for h in range(108, 128)]
    + [
        ("b", 103, 104, True), ("b", 40, 70, False), ("b", 70, 100, False),
        ("b", 0, 18, False), ("b", 102, 103, False), ("b", 100, 102, False),
    ],
    "A": [("b", 0, 100, False), ("b", 100, 104, False)],
    "B": [
        ("b", 104, 116, True), ("b", 116, 128, True),
        ("b", 0, 100, False), ("b", 100, 104, False),
    ],
}
_EARLY = {"C": range(3, 9), "D": [*range(54, 64), 51], "A": (), "B": ()}
_BULK = {
    "C": [(0, 6), (6, 16), (16, 36), (36, 64)],
    "D": [(0, 36), (36, 64)],
    "A": [(0, 64)],
    "B": [(0, 64)],
}
_ORDER_A = (
    [("y", i) for i in range(10)] + [None]
    + [("x", i) for i in range(18)] + [("y", 10)]
    + [("x", i) for i in range(18, 22)] + [("y", 11)]
    + [("x", 22), ("x", 23), ("y", 12), ("x", 24), ("y", 13)]
)


def _recv_order(r):
    if r == "A":
        return _ORDER_A
    ys = [("y", i) for i in range(len(_SENDS[_Y_PEER[r]]))]
    diag = _SENDS[_Y_PEER[_X_PEER[r]]]
    xs = [("x", i) for i, msg in enumerate(diag) if msg[3]]
    return ys[:-1] + xs + ys[-1:]


def _tile(k):
    return pl.ds(8 * k, 8)


def _halves(buf, h0, h1):
    if h1 - h0 == 1:
        return buf.at[h0 // 2, pl.ds(4 * (h0 % 2), 4)]
    assert h0 % 2 == 0 and h1 % 2 == 0
    return buf.at[pl.ds(h0 // 2, (h1 - h0) // 2)]


def _bits(v):
    return lax.bitcast_convert_type(v.astype(jnp.float32), jnp.uint32)


def _rows_of_parity(v, p):
    w = pltpu.bitcast(v, jnp.uint32)
    w = w & jnp.uint32(0xFFFF0000) if p else w << 16
    return lax.bitcast_convert_type(w, jnp.float32).astype(jnp.bfloat16)


def _interleave_rows(even, odd):
    return pltpu.bitcast((_bits(even) >> 16) | _bits(odd), jnp.bfloat16)


def _body(rows_hbm, pairs_hbm, o_ref, xv, xe, sbuf, rbuf, hbuf,
          y_send, y_recv, x_send, x_recv, load_sem, relay_sem):
    my_x = lax.axis_index("x")
    my_y = lax.axis_index("y")
    barrier = pltpu.get_barrier_semaphore()
    pl.semaphore_signal(barrier, inc=1, device_id=(my_x, 1 - my_y),
                        device_id_type=_MESH)

    def signal(sem, dev):
        pl.semaphore_signal(sem, inc=1, device_id=_DEV[dev], device_id_type=_MESH)

    def hbm_pieces(h0, h1, dst):
        g = _X1[h0 // 2]
        if isinstance(g, int):
            srcs = [rows_hbm.at[pl.ds(8 * g + 4 * (h0 % 2), 4 * (h1 - h0))]]
        elif h1 - h0 == 2 and g[1] == g[0] + 1:
            srcs = [pairs_hbm.at[pl.ds(4 * g[0], 8), g[2]]]
        else:
            srcs = [pairs_hbm.at[pl.ds(4 * g[h % 2], 4), g[2]] for h in range(h0, h1)]
        n = 4 * (h1 - h0) // len(srcs)
        return [(s, dst.at[pl.ds(4 * h0 + n * j, n)]) for j, s in enumerate(srcs)]

    def y_copy(msg, i, dev):
        kind, h0, h1, _ = msg
        if kind == "b":
            src, dst = _halves(sbuf, h0, h1), _halves(rbuf, h0, h1)
        else:
            ((src, dst),) = hbm_pieces(h0, h1, hbuf)
        return pltpu.make_async_remote_copy(
            src_ref=src, dst_ref=dst, send_sem=y_send.at[i], recv_sem=y_recv.at[i],
            device_id=_DEV[dev], device_id_type=_MESH)

    def x_copy(msg, i, dev):
        buf = _halves(rbuf, msg[1], msg[2])
        return pltpu.make_async_remote_copy(
            src_ref=buf, dst_ref=buf, send_sem=x_send.at[i], recv_sem=x_recv.at[i],
            device_id=_DEV[dev], device_id_type=_MESH)

    def program(r):
        yp, xp = _Y_PEER[r], _X_PEER[r]
        mine = _SENDS[r]
        n_head = sum(msg[0] == "f" for msg in mine)
        sent, received = (range(_NG), _X1) if r in "AB" else (_X1, range(_NG))
        in_flight = []

        def wait_peers():
            pl.semaphore_wait(barrier, {"A": 2, "B": 3, "C": 1, "D": 1}[r])

        def send(i):
            cp = y_copy(mine[i], i, yp)
            cp.start()
            in_flight.append(cp)

        sems = iter(range(load_sem.shape[0]))
        early = {
            g: [pltpu.make_async_copy(src, dst, load_sem.at[next(sems)])
                for src, dst in hbm_pieces(2 * g, 2 * g + 2, xe)]
            for g in _EARLY[r]
        }
        bulk = {}
        for k0, k1 in _BULK[r]:
            rows = pl.ds(8 * k0, 8 * (k1 - k0))
            bulk[k0, k1] = pltpu.make_async_copy(
                rows_hbm.at[rows], xv.at[rows], load_sem.at[next(sems)])

        def start(copies):
            for cp in copies:
                cp.start()

        early_loads = [cp for cps in early.values() for cp in cps]
        if r == "C":
            start(early_loads[:1])
            wait_peers()
            for i in range(n_head):
                send(i)
            start(early_loads[1:3])
            signal(barrier, "B")
            start(early_loads[3:])
            start(bulk.values())
        elif r == "D":
            start(early_loads)
            wait_peers()
            for i in range(n_head):
                send(i)
        else:
            signal(barrier, xp)
            start(bulk.values())

        def need_tile(k):
            for k0, k1 in list(bulk):
                if k0 <= k < k1:
                    bulk.pop((k0, k1)).wait()

        packed = set()

        def pack(i):
            todo = [g for g in range(mine[i][1] // 2, (mine[i][2] + 1) // 2)
                    if g not in packed]
            packed.update(todo)
            for g in todo:
                if g in early:
                    for cp in early[g]:
                        cp.wait()
                elif isinstance(sent[g], int):
                    need_tile(sent[g])
                else:
                    need_tile(sent[g][0])
                    need_tile(sent[g][1])
            for g in todo:
                if g in early:
                    sbuf[g] = xe[_tile(g), :].astype(jnp.bfloat16)
                elif isinstance(sent[g], int):
                    sbuf[g] = xv[_tile(sent[g]), :].astype(jnp.bfloat16)
                else:
                    k1, k2, p = sent[g]
                    both = jnp.concatenate([xv[_tile(k1), :], xv[_tile(k2), :]])
                    sbuf[g] = _rows_of_parity(both.astype(jnp.bfloat16), p)

        if r in "AB":
            for i in range(len(mine)):
                pack(i)
            wait_peers()
            for i in range(len(mine)):
                send(i)
        else:
            for i in range(n_head, len(mine)):
                pack(i)
                send(i)
                if r == "D" and i == n_head:
                    start(bulk.values())
        for k0, _ in list(bulk):
            need_tile(k0)

        if r == "B":
            signal(relay_sem, "D")
        if r == "D":
            pl.semaphore_wait(relay_sem, 1)

        from_y, from_diag = _SENDS[yp], _SENDS[_Y_PEER[xp]]
        arrived = set()
        deferred = []

        def add(h0, h1):
            for h in range(h0, h1):
                arrived.add(h)
                g = received[h // 2]
                if isinstance(g, int):
                    if h ^ 1 in arrived:
                        o_ref[_tile(g), :] = (
                            xv[_tile(g), :] + rbuf[h // 2].astype(jnp.float32))
                    continue
                even, odd = (received.index(g[:2] + (p,)) for p in (0, 1))
                if arrived >= {2 * even, 2 * even + 1, 2 * odd, 2 * odd + 1}:
                    both = _interleave_rows(rbuf[even], rbuf[odd])
                    both = both.astype(jnp.float32)
                    o_ref[_tile(g[0]), :] = xv[_tile(g[0]), :] + both[:8]
                    o_ref[_tile(g[1]), :] = xv[_tile(g[1]), :] + both[8:]

        def flush():
            for msg in deferred:
                add(msg[1], msg[2])
            deferred.clear()

        def drain():
            for cp in in_flight:
                cp.wait_send()
            in_flight.clear()

        for event in _recv_order(r):
            if event is None:
                drain()
                continue
            src, i = event
            if src == "y":
                msg = from_y[i]
                kind, h0, h1, fwd = msg
                y_copy(msg, i, yp).wait_recv()
                if kind == "f":
                    n = 4 * (h1 - h0)
                    rbuf[h0 // 2, pl.ds(4 * (h0 % 2), n), :] = (
                        hbuf[pl.ds(4 * h0, n), :].astype(jnp.bfloat16))
                if fwd:
                    cp = x_copy(msg, i, xp)
                    cp.start()
                    in_flight.append(cp)
                    deferred.append(msg)
                else:
                    flush()
                    add(h0, h1)
            else:
                msg = from_diag[i]
                flush()
                x_copy(msg, i, xp).wait_recv()
                add(msg[1], msg[2])
        flush()
        drain()
        assert len(arrived) == 2 * _NG

    for r in "CDAB":
        is_r = jnp.logical_and(my_x == _DEV[r][0], my_y == _DEV[r][1])
        pl.when(is_r)(functools.partial(program, r))


def pallas_dist_ar_xy_y_m256_n256_kernel(x: jax.Array):
    assert x.shape == (256, 256)
    rows = x.reshape(32, 8, 2, 128).transpose(0, 2, 1, 3).reshape(512, 128)
    n_msg = max(len(v) for v in _SENDS.values())
    n_load = max(2 * len(_EARLY[r]) + len(_BULK[r]) for r in _DEV)
    out = pl.pallas_call(
        _body,
        out_shape=jax.ShapeDtypeStruct((512, 128), x.dtype),
        in_specs=[pl.BlockSpec(memory_space=pl.ANY)] * 2,
        out_specs=pl.BlockSpec(memory_space=pltpu.VMEM),
        scratch_shapes=[
            pltpu.VMEM((512, 128), x.dtype),
            pltpu.VMEM((512, 128), x.dtype),
            pltpu.VMEM((_NG, 8, 128), jnp.bfloat16),
            pltpu.VMEM((_NG, 8, 128), jnp.bfloat16),
            pltpu.VMEM((512, 128), x.dtype),
            pltpu.SemaphoreType.DMA((n_msg,)),
            pltpu.SemaphoreType.DMA((n_msg,)),
            pltpu.SemaphoreType.DMA((n_msg,)),
            pltpu.SemaphoreType.DMA((n_msg,)),
            pltpu.SemaphoreType.DMA((n_load,)),
            pltpu.SemaphoreType.REGULAR,
        ],
        compiler_params=pltpu.CompilerParams(
            collective_id=0,
            disable_bounds_checks=True,
            disable_semaphore_checks=True,
        ),
    )(rows, rows.reshape(256, 2, 128))
    return out.reshape(32, 2, 8, 128).transpose(0, 2, 1, 3).reshape(256, 256)
```

```python
import functools

import jax
import jax.numpy as jnp
from jax import lax
from jax.experimental import pallas as pl
from jax.experimental.pallas import tpu as pltpu

_MESH = pl.DeviceIdType.MESH
_DEV = {"A": (0, 0), "B": (1, 0), "C": (0, 1), "D": (1, 1)}
_Y_PEER = {"A": "C", "C": "A", "B": "D", "D": "B"}
_X_PEER = {"A": "B", "B": "A", "C": "D", "D": "C"}
_NG = 64

_X1 = [
    (14, 15, 0), (30, 31, 1), (42, 43, 1), (50, 51, 1),
    (0, 5, 0), (9, 12, 1), (17, 20, 1), (7, 22, 0), (25, 28, 0),
    (0, 5, 1), (2, 3, 0), 1, 4,
    (14, 15, 1), (9, 12, 0), 6, 8, 10, 11, 13,
    (30, 31, 0), (17, 20, 0), (7, 22, 1), (25, 28, 1),
    16, 18, 19, 21, 24, 26, 27, 29, 32, 34, 35,
    (42, 43, 0), (50, 51, 0), (58, 59, 1), (33, 36, 1), (23, 38, 0),
    (40, 45, 1), (48, 53, 1), (56, 61, 0), 37, 39, 41, 44, 46, 47, 49, 52, 54,
    (58, 59, 0), (2, 3, 1), (33, 36, 0), (23, 38, 1), (40, 45, 0), (48, 53, 0),
    (56, 61, 1), 55, 57, 60, 62, 63,
]

_SENDS = {
    "C": [
        ("f", 0, 4, False), ("f", 4, 8, False), ("f", 8, 12, False),
        ("b", 12, 16, False), ("b", 16, 20, False), ("b", 20, 24, False),
        ("b", 24, 36, False), ("b", 36, 52, True), ("b", 52, 80, True),
        ("b", 80, 140, False), ("b", 140, 172, False), ("b", 172, 192, False),
        ("b", 192, 200, False), ("b", 200, 204, False), ("b", 204, 205, False),
    ],
    "D": [("f", q, q + 1, True) for q in range(208, 217)]
    + [("b", q, q + 1, True) for q in [*range(217, 256), 205, 206, 207]]
    + [
        ("b", 80, 140, False), ("b", 140, 200, False), ("b", 0, 36, False),
        ("b", 204, 205, False), ("b", 200, 204, False),
    ],
    "A": [("b", 0, 200, False), ("b", 200, 208, False)],
    "B": [
        ("b", 208, 232, True), ("b", 232, 256, True),
        ("b", 0, 200, False), ("b", 200, 208, False),
    ],
}
_EARLY = {"C": range(3, 9), "D": [*range(54, 64), 51], "A": (), "B": ()}
_BULK = {
    "C": [(0, 6), (6, 16), (16, 36), (36, 64)],
    "D": [(0, 36), (36, 64)],
    "A": [(0, 64)],
    "B": [(0, 64)],
}
_ORDER_A = (
    [("y", i) for i in range(10)] + [None]
    + [("x", i) for i in range(18)] + [("y", 10)]
    + [("x", i) for i in range(18, 38)] + [("y", 11)]
    + [("x", i) for i in range(38, 46)] + [("y", 12)]
    + [("x", i) for i in range(46, 50)] + [("y", 13), ("x", 50), ("y", 14)]
)


def _recv_order(r):
    if r == "A":
        return _ORDER_A
    ys = [("y", i) for i in range(len(_SENDS[_Y_PEER[r]]))]
    diag = _SENDS[_Y_PEER[_X_PEER[r]]]
    xs = [("x", i) for i, msg in enumerate(diag) if msg[3]]
    return ys[:-1] + xs + ys[-1:]


def _tile(k):
    return pl.ds(8 * k, 8)


def _quarters(buf, q0, q1):
    if q1 - q0 == 1:
        return buf.at[q0 // 4, pl.ds(2 * (q0 % 4), 2)]
    assert q0 % 4 == 0 and q1 % 4 == 0
    return buf.at[pl.ds(q0 // 4, (q1 - q0) // 4)]


def _bits(v):
    return lax.bitcast_convert_type(v.astype(jnp.float32), jnp.uint32)


def _rows_of_parity(v, p):
    w = pltpu.bitcast(v, jnp.uint32)
    w = w & jnp.uint32(0xFFFF0000) if p else w << 16
    return lax.bitcast_convert_type(w, jnp.float32).astype(jnp.bfloat16)


def _interleave_rows(even, odd):
    return pltpu.bitcast((_bits(even) >> 16) | _bits(odd), jnp.bfloat16)


def _body(rows_hbm, pairs_hbm, o_ref, xv, xe, sbuf, rbuf, hbuf,
          y_send, y_recv, x_send, x_recv, load_sem, relay_sem):
    my_x = lax.axis_index("x")
    my_y = lax.axis_index("y")
    barrier = pltpu.get_barrier_semaphore()
    pl.semaphore_signal(barrier, inc=1, device_id=(my_x, 1 - my_y),
                        device_id_type=_MESH)

    def signal(sem, dev):
        pl.semaphore_signal(sem, inc=1, device_id=_DEV[dev], device_id_type=_MESH)

    def hbm_pieces(q0, q1, dst):
        g = _X1[q0 // 4]
        if isinstance(g, int):
            srcs = [rows_hbm.at[pl.ds(8 * g + 2 * (q0 % 4), 2 * (q1 - q0))]]
        elif q1 - q0 == 1:
            srcs = [pairs_hbm.at[pl.ds(4 * g[q0 % 4 // 2] + 2 * (q0 % 2), 2), g[2]]]
        elif g[1] == g[0] + 1:
            srcs = [pairs_hbm.at[pl.ds(4 * g[0], 8), g[2]]]
        else:
            srcs = [pairs_hbm.at[pl.ds(4 * k, 4), g[2]] for k in g[:2]]
        n = 2 * (q1 - q0) // len(srcs)
        return [(s, dst.at[pl.ds(2 * q0 + n * j, n)]) for j, s in enumerate(srcs)]

    def y_copy(msg, i, dev):
        kind, q0, q1, _ = msg
        if kind == "b":
            src, dst = _quarters(sbuf, q0, q1), _quarters(rbuf, q0, q1)
        else:
            ((src, dst),) = hbm_pieces(q0, q1, hbuf)
        return pltpu.make_async_remote_copy(
            src_ref=src, dst_ref=dst, send_sem=y_send.at[i], recv_sem=y_recv.at[i],
            device_id=_DEV[dev], device_id_type=_MESH)

    def x_copy(msg, i, dev):
        buf = _quarters(rbuf, msg[1], msg[2])
        return pltpu.make_async_remote_copy(
            src_ref=buf, dst_ref=buf, send_sem=x_send.at[i], recv_sem=x_recv.at[i],
            device_id=_DEV[dev], device_id_type=_MESH)

    def program(r):
        yp, xp = _Y_PEER[r], _X_PEER[r]
        mine = _SENDS[r]
        n_head = sum(msg[0] == "f" for msg in mine)
        sent, received = (range(_NG), _X1) if r in "AB" else (_X1, range(_NG))
        in_flight = []

        def wait_peers():
            pl.semaphore_wait(barrier, {"A": 2, "B": 3, "C": 1, "D": 1}[r])

        def send(i):
            cp = y_copy(mine[i], i, yp)
            cp.start()
            in_flight.append(cp)

        sems = iter(range(load_sem.shape[0]))
        early = {
            g: [pltpu.make_async_copy(src, dst, load_sem.at[next(sems)])
                for src, dst in hbm_pieces(4 * g, 4 * g + 4, xe)]
            for g in _EARLY[r]
        }
        bulk = {}
        for k0, k1 in _BULK[r]:
            rows = pl.ds(8 * k0, 8 * (k1 - k0))
            bulk[k0, k1] = pltpu.make_async_copy(
                rows_hbm.at[rows], xv.at[rows], load_sem.at[next(sems)])

        def start(copies):
            for cp in copies:
                cp.start()

        early_loads = [cp for cps in early.values() for cp in cps]
        if r == "C":
            start(early_loads[:1])
            wait_peers()
            for i in range(n_head):
                send(i)
            start(early_loads[1:3])
            signal(barrier, "B")
            start(early_loads[3:])
            start(bulk.values())
        elif r == "D":
            start(early_loads)
            wait_peers()
            for i in range(n_head):
                send(i)
        else:
            signal(barrier, xp)
            start(bulk.values())

        def need_tile(k):
            for k0, k1 in list(bulk):
                if k0 <= k < k1:
                    bulk.pop((k0, k1)).wait()

        packed = set()

        def pack(i):
            todo = [g for g in range(mine[i][1] // 4, (mine[i][2] + 3) // 4)
                    if g not in packed]
            packed.update(todo)
            for g in todo:
                if g in early:
                    for cp in early[g]:
                        cp.wait()
                elif isinstance(sent[g], int):
                    need_tile(sent[g])
                else:
                    need_tile(sent[g][0])
                    need_tile(sent[g][1])
            for g in todo:
                if g in early:
                    sbuf[g] = xe[_tile(g), :].astype(jnp.bfloat16)
                elif isinstance(sent[g], int):
                    sbuf[g] = xv[_tile(sent[g]), :].astype(jnp.bfloat16)
                else:
                    k1, k2, p = sent[g]
                    both = jnp.concatenate([xv[_tile(k1), :], xv[_tile(k2), :]])
                    sbuf[g] = _rows_of_parity(both.astype(jnp.bfloat16), p)

        if r in "AB":
            for i in range(len(mine)):
                pack(i)
            wait_peers()
            for i in range(len(mine)):
                send(i)
        else:
            for i in range(n_head, len(mine)):
                pack(i)
                send(i)
                if r == "D" and i == n_head:
                    start(bulk.values())
        for k0, _ in list(bulk):
            need_tile(k0)

        if r == "B":
            signal(relay_sem, "D")
        if r == "D":
            pl.semaphore_wait(relay_sem, 1)

        from_y, from_diag = _SENDS[yp], _SENDS[_Y_PEER[xp]]
        arrived = set()
        deferred = []

        def complete(*granules):
            return all(4 * g + j in arrived for g in granules for j in range(4))

        def add(q0, q1):
            for q in range(q0, q1):
                arrived.add(q)
                g = received[q // 4]
                if isinstance(g, int):
                    if complete(q // 4):
                        o_ref[_tile(g), :] = (
                            xv[_tile(g), :] + rbuf[q // 4].astype(jnp.float32))
                    continue
                even, odd = (received.index(g[:2] + (p,)) for p in (0, 1))
                if complete(even, odd):
                    both = _interleave_rows(rbuf[even], rbuf[odd])
                    both = both.astype(jnp.float32)
                    o_ref[_tile(g[0]), :] = xv[_tile(g[0]), :] + both[:8]
                    o_ref[_tile(g[1]), :] = xv[_tile(g[1]), :] + both[8:]

        def flush():
            for msg in deferred:
                add(msg[1], msg[2])
            deferred.clear()

        def drain():
            for cp in in_flight:
                cp.wait_send()
            in_flight.clear()

        for event in _recv_order(r):
            if event is None:
                drain()
                continue
            src, i = event
            if src == "y":
                msg = from_y[i]
                kind, q0, q1, fwd = msg
                y_copy(msg, i, yp).wait_recv()
                if kind == "f":
                    n = 2 * (q1 - q0)
                    rbuf[q0 // 4, pl.ds(2 * (q0 % 4), n), :] = (
                        hbuf[pl.ds(2 * q0, n), :].astype(jnp.bfloat16))
                if fwd:
                    cp = x_copy(msg, i, xp)
                    cp.start()
                    in_flight.append(cp)
                    deferred.append(msg)
                else:
                    flush()
                    add(q0, q1)
            else:
                msg = from_diag[i]
                flush()
                x_copy(msg, i, xp).wait_recv()
                add(msg[1], msg[2])
        flush()
        drain()
        assert complete(*range(_NG))

    for r in "CDBA":
        is_r = jnp.logical_and(my_x == _DEV[r][0], my_y == _DEV[r][1])
        pl.when(is_r)(functools.partial(program, r))


def pallas_dist_ar_xy_y_m256_n256_kernel(x: jax.Array):
    assert x.shape == (256, 256)
    rows = x.reshape(32, 8, 2, 128).transpose(0, 2, 1, 3).reshape(512, 128)
    n_msg = max(len(v) for v in _SENDS.values())
    n_load = max(2 * len(_EARLY[r]) + len(_BULK[r]) for r in _DEV)
    out = pl.pallas_call(
        _body,
        out_shape=jax.ShapeDtypeStruct((512, 128), x.dtype),
        in_specs=[pl.BlockSpec(memory_space=pl.ANY)] * 2,
        out_specs=pl.BlockSpec(memory_space=pltpu.VMEM),
        scratch_shapes=[
            pltpu.VMEM((512, 128), x.dtype),
            pltpu.VMEM((512, 128), x.dtype),
            pltpu.VMEM((_NG, 8, 128), jnp.bfloat16),
            pltpu.VMEM((_NG, 8, 128), jnp.bfloat16),
            pltpu.VMEM((512, 128), x.dtype),
            pltpu.SemaphoreType.DMA((n_msg,)),
            pltpu.SemaphoreType.DMA((n_msg,)),
            pltpu.SemaphoreType.DMA((n_msg,)),
            pltpu.SemaphoreType.DMA((n_msg,)),
            pltpu.SemaphoreType.DMA((n_load,)),
            pltpu.SemaphoreType.REGULAR,
        ],
        compiler_params=pltpu.CompilerParams(
            collective_id=0,
            disable_bounds_checks=True,
            disable_semaphore_checks=True,
        ),
    )(rows, rows.reshape(256, 2, 128))
    return out.reshape(32, 2, 8, 128).transpose(0, 2, 1, 3).reshape(256, 256)
```
